```python
import numpy as np

kernel_name = "dist_ar_xy_y_m1024_n512"

def setup_inputs():
    return {"x": np.random.randn(2048, 512).astype(np.float32)}

def reference(x: np.ndarray) -> np.ndarray:
    return x.reshape(2, 1024, 512).sum(axis=0)
```

```python
import jax
import jax.numpy as jnp
from jax import lax
from jax.experimental import pallas as pl
from jax.experimental.pallas import tpu as pltpu

M, N = 1024, 512
B = 8
R = 472
CW = 256
WIN = 16
NB, NCW = R // B, N // CW
T0 = M - R
ZL = T0 - B
LOADS = (8, 24, 64, 128, R - 224, T0 - R, R)
DIRECT = ((R, ZL - B - R), (ZL - B, B))
XGROUPS = (32,) * 14 + (B,) * 3
LAG = T0 - R + 2 * B
MESH = pl.DeviceIdType.MESH

assert sum(LOADS) == M and sum(XGROUPS) == R


def _body(x_hbm, out_ref, xv, sendb, other, z32, ld_sems, send_sems, yrecv_sems,
          xrecv_sems, xready):
    mx = lax.axis_index("x")
    my = lax.axis_index("y")
    ynbr = (mx, 1 - my)
    xnbr = (1 - mx, my)
    is00 = jnp.logical_and(mx == 0, my == 0)
    is01 = jnp.logical_and(mx == 0, my == 1)
    is11 = jnp.logical_and(mx == 1, my == 1)

    def global_rows(l, n):
        if l < R:
            return pl.ds(pl.multiple_of(mx * R + l, B), n)
        if l < T0:
            return pl.ds(l + R, n)
        return pl.ds(pl.multiple_of((1 - mx) * R + (l - T0), B), n)

    def remote(src, dst, send_sem, recv_sem, device):
        return pltpu.make_async_remote_copy(
            src_ref=src, dst_ref=dst, send_sem=send_sem, recv_sem=recv_sem,
            device_id=device, device_id_type=MESH)

    def piece(ref, l, c):
        return ref.at[pl.ds(l, B), pl.ds(c * CW, CW)]

    group_start = [sum(XGROUPS[:g]) for g in range(len(XGROUPS))]
    group_of = [g for g, n in enumerate(XGROUPS) for _ in range(n // B)]

    def y_piece(b, c):
        return remote(piece(sendb, b * B, c), piece(other, b * B, c),
                      send_sems.at[0], yrecv_sems.at[b * NCW + c], ynbr)

    def y_direct(k):
        rows = pl.ds(*DIRECT[k])
        return remote(sendb.at[rows], other.at[rows],
                      send_sems.at[0], yrecv_sems.at[NB * NCW + k], ynbr)

    def x_piece(b, c):
        return remote(piece(other, b * B, c), piece(other, T0 + b * B, c),
                      send_sems.at[1], xrecv_sems.at[group_of[b]], xnbr)

    zrows = pl.ds(ZL, B)
    zsem = yrecv_sems.at[NB * NCW + len(DIRECT)]

    def z_f32():
        return remote(x_hbm.at[global_rows(ZL, B)], z32, send_sems.at[2], zsem, ynbr)

    def z_bf16():
        return remote(sendb.at[zrows], other.at[zrows], send_sems.at[2], zsem, ynbr)

    def wait_total(ref, sem):
        pltpu.make_async_copy(ref, ref, sem).wait()

    load_start = [sum(LOADS[:i]) for i in range(len(LOADS))]
    loads = [
        pltpu.make_async_copy(x_hbm.at[global_rows(l, n)], xv.at[pl.ds(l, n)], ld_sems.at[i])
        for i, (l, n) in enumerate(zip(load_start, LOADS))
    ]
    loads[0].start()

    bar = pltpu.get_barrier_semaphore()
    pl.semaphore_signal(bar, inc=1, device_id=ynbr, device_id_type=MESH)

    @pl.when(jnp.logical_not(is11))
    def _():
        pl.semaphore_signal(bar, inc=1, device_id=xnbr, device_id_type=MESH)

    @pl.when(is01)
    def _():
        pl.semaphore_wait(bar, 1)
        z_f32().start()

    for cp in loads[1:]:
        cp.start()

    def cast(l, n):
        sendb[pl.ds(l, n), :] = xv[pl.ds(l, n), :].astype(jnp.bfloat16)

    def send_step(b):
        if b * B in load_start and b <= NB:
            loads[load_start.index(b * B)].wait()
        if b < NB:
            cast(b * B, B)
            if b == 0:
                @pl.when(jnp.logical_not(is01))
                def _():
                    pl.semaphore_wait(bar, 2)

            for c in range(NCW):
                y_piece(b, c).start()
            if b == 0:
                @pl.when(is11)
                def _():
                    pl.semaphore_signal(xready, inc=1, device_id=xnbr, device_id_type=MESH)
        elif b == NB:
            for k in range(len(DIRECT)):
                cast(*DIRECT[k])
                y_direct(k).start()

            @pl.when(jnp.logical_not(is01))
            def _():
                cast(ZL, B)
                z_bf16().start()

    def finish(l, n):
        rows = pl.ds(l, n)
        out_ref[global_rows(l, n), :] = xv[rows, :] + other[rows, :].astype(jnp.float32)

    consumed = [0]

    def consume_x(y_rows_done):
        while consumed[0] < len(XGROUPS):
            g = consumed[0]
            if group_start[g] + XGROUPS[g] + LAG > y_rows_done:
                break
            if g == 0:
                loads[-1].wait()
            wait_total(other.at[pl.ds(T0 + group_start[g], XGROUPS[g])], xrecv_sems.at[g])
            finish(T0 + group_start[g], XGROUPS[g])
            consumed[0] += 1

    for b in range(WIN):
        send_step(b)

    @pl.when(is01)
    def _():
        pl.semaphore_wait(xready, 1)

    for b in range(NB):
        for c in range(NCW):
            y_piece(b, c).wait_recv()
            x_piece(b, c).start()
        send_step(b + WIN)
        finish(b * B, B)
        consume_x((b + 1) * B)

    @pl.when(is00)
    def _():
        z_f32().wait_recv()
        out_ref[global_rows(ZL, B), :] = xv[zrows, :] + z32[...]

    for k, (l, n) in enumerate(DIRECT):
        if k == len(DIRECT) - 1:
            wait_total(other.at[pl.ds(0, R)], send_sems.at[1])
            wait_total(sendb.at[pl.ds(0, ZL)], send_sems.at[0])

            @pl.when(is01)
            def _():
                z_f32().wait_send()

            @pl.when(jnp.logical_not(is01))
            def _():
                z_bf16().wait_send()

        y_direct(k).wait_recv()
        finish(l, n)
        consume_x(l + n)
    consume_x(2 * M)

    @pl.when(jnp.logical_not(is00))
    def _():
        z_bf16().wait_recv()
        finish(ZL, B)


def pallas_dist_ar_xy_y_m1024_n512_kernel(x: jax.Array):
    return pl.pallas_call(
        _body,
        out_shape=jax.ShapeDtypeStruct((M, N), jnp.float32),
        in_specs=[pl.BlockSpec(memory_space=pl.ANY)],
        out_specs=pl.BlockSpec(memory_space=pltpu.VMEM),
        scratch_shapes=[
            pltpu.VMEM((M, N), jnp.float32),
            pltpu.VMEM((T0, N), jnp.bfloat16),
            pltpu.VMEM((M, N), jnp.bfloat16),
            pltpu.VMEM((B, N), jnp.float32),
            pltpu.SemaphoreType.DMA((len(LOADS),)),
            pltpu.SemaphoreType.DMA((3,)),
            pltpu.SemaphoreType.DMA((NB * NCW + len(DIRECT) + 1,)),
            pltpu.SemaphoreType.DMA((len(XGROUPS),)),
            pltpu.SemaphoreType.REGULAR,
        ],
        compiler_params=pltpu.CompilerParams(
            collective_id=0,
            disable_semaphore_checks=True,
        ),
    )(x)
```

```python
import jax
import jax.numpy as jnp
from jax import lax
from jax.experimental import pallas as pl
from jax.experimental.pallas import tpu as pltpu

M, N = 1024, 512
B, CW = 8, 128
R = 472
NB, NCW = R // B, N // CW
T0 = M - R
ZL = T0 - B
ZC = 384
WIN = 12
LAG = (T0 - R) // B + 2
LOADS = (B, 24, 64, 128, R - 224, T0 - R, R)
DIRECT = ((R, ZL - B - R), (ZL - B, B))
XGROUPS = (4,) * 14 + (1,) * 3
MESH = pl.DeviceIdType.MESH

assert sum(LOADS) == M and sum(XGROUPS) == NB


def _body(x_hbm, out_ref, xv, sendb, other, tile0, z32, ld_sems, send_sems,
          yrecv_sems, xrecv_sems, xready):
    mx = lax.axis_index("x")
    my = lax.axis_index("y")
    ynbr = (mx, 1 - my)
    xnbr = (1 - mx, my)
    is00 = jnp.logical_and(mx == 0, my == 0)
    is01 = jnp.logical_and(mx == 0, my == 1)
    is11 = jnp.logical_and(mx == 1, my == 1)

    def global_rows(l, n):
        if l < R:
            return pl.ds(pl.multiple_of(mx * R + l, B), n)
        if l < T0:
            return pl.ds(l + R, n)
        return pl.ds(pl.multiple_of((1 - mx) * R + (l - T0), B), n)

    def remote(src, dst, send_sem, recv_sem, device):
        return pltpu.make_async_remote_copy(
            src_ref=src, dst_ref=dst, send_sem=send_sem, recv_sem=recv_sem,
            device_id=device, device_id_type=MESH)

    def wait_total(ref, sem):
        pltpu.make_async_copy(ref, ref, sem).wait()

    group_end = [sum(XGROUPS[:g + 1]) for g in range(len(XGROUPS))]
    group_of = [g for g, n in enumerate(XGROUPS) for _ in range(n)]

    def piece(ref, l, c):
        return ref.at[pl.ds(l, B), pl.ds(c * CW, CW)]

    def y_piece(b, c):
        return remote(piece(sendb, b * B, c), piece(other, b * B, c),
                      send_sems.at[0], yrecv_sems.at[b * NCW + c], ynbr)

    def x_piece(b, c):
        return remote(piece(other, b * B, c), piece(other, T0 + b * B, c),
                      send_sems.at[1], xrecv_sems.at[group_of[b]], xnbr)

    def y_direct(k):
        rows = pl.ds(*DIRECT[k])
        return remote(sendb.at[rows], other.at[rows],
                      send_sems.at[0], yrecv_sems.at[NB * NCW + k], ynbr)

    zrows, zhead, ztail = pl.ds(ZL, B), pl.ds(0, ZC), pl.ds(ZC, N - ZC)
    zsem = NB * NCW + len(DIRECT)

    def z_head_f32():
        return remote(x_hbm.at[global_rows(ZL, B), zhead], z32,
                      send_sems.at[2], yrecv_sems.at[zsem], ynbr)

    def z_head_bf16():
        return remote(sendb.at[zrows, zhead], other.at[zrows, zhead],
                      send_sems.at[2], yrecv_sems.at[zsem], ynbr)

    def z_tail():
        return remote(sendb.at[zrows, ztail], other.at[zrows, ztail],
                      send_sems.at[3], yrecv_sems.at[zsem + 1], ynbr)

    load_tile0 = pltpu.make_async_copy(
        x_hbm.at[global_rows(0, B), pl.ds(0, CW)], tile0, ld_sems.at[len(LOADS)])
    load_start = [sum(LOADS[:i]) for i in range(len(LOADS))]
    loads = [
        pltpu.make_async_copy(x_hbm.at[global_rows(l, n)], xv.at[pl.ds(l, n)], ld_sems.at[i])
        for i, (l, n) in enumerate(zip(load_start, LOADS))
    ]
    load_tile0.start()
    loads[0].start()

    bar = pltpu.get_barrier_semaphore()
    pl.semaphore_signal(bar, inc=1, device_id=ynbr, device_id_type=MESH)

    @pl.when(jnp.logical_not(is11))
    def _():
        pl.semaphore_signal(bar, inc=1, device_id=xnbr, device_id_type=MESH)

    @pl.when(is01)
    def _():
        pl.semaphore_wait(bar, 1)
        z_head_f32().start()

    for cp in loads[1:]:
        cp.start()

    @pl.when(jnp.logical_not(is01))
    def _():
        pl.semaphore_wait(bar, 2)

    def cast(l, n, cols=slice(None)):
        sendb[pl.ds(l, n), cols] = xv[pl.ds(l, n), cols].astype(jnp.bfloat16)

    def send_step(b):
        if b == 0:
            load_tile0.wait()
            sendb[pl.ds(0, B), pl.ds(0, CW)] = tile0[...].astype(jnp.bfloat16)
            y_piece(0, 0).start()
        if b <= NB and b * B in load_start:
            loads[load_start.index(b * B)].wait()
        if b < NB:
            first = 1 if b == 0 else 0
            cast(b * B, B, pl.ds(first * CW, N - first * CW))
            for c in range(first, NCW):
                y_piece(b, c).start()
        elif b == NB:
            for k in range(len(DIRECT)):
                cast(*DIRECT[k])
                y_direct(k).start()
            cast(ZL, B)
            z_tail().start()

            @pl.when(jnp.logical_not(is01))
            def _():
                z_head_bf16().start()

    def finish(l, n, cols=slice(None)):
        rows = pl.ds(l, n)
        out_ref[global_rows(l, n), cols] = (
            xv[rows, cols] + other[rows, cols].astype(jnp.float32))

    x_done = [0]

    def consume_x(y_blocks, limit=NB):
        while limit and x_done[0] < NB:
            j = x_done[0]
            g = group_of[j]
            if group_end[g] + LAG > y_blocks:
                break
            if j == 0:
                loads[-1].wait()
            if j == group_end[g] - XGROUPS[g]:
                wait_total(other.at[pl.ds(T0 + j * B, XGROUPS[g] * B)], xrecv_sems.at[g])
            finish(T0 + j * B, B)
            x_done[0] += 1
            limit -= 1

    send_step(0)

    @pl.when(is11)
    def _():
        pl.semaphore_signal(xready, inc=1, device_id=xnbr, device_id_type=MESH)

    for b in range(1, WIN):
        send_step(b)

    @pl.when(is01)
    def _():
        pl.semaphore_wait(xready, 1)

    for b in range(NB):
        for c in range(NCW):
            y_piece(b, c).wait_recv()
            x_piece(b, c).start()
        send_step(b + WIN)
        finish(b * B, B)
        consume_x(b, limit=1)

    for k, (l, n) in enumerate(DIRECT):
        if k == len(DIRECT) - 1:
            wait_total(other.at[pl.ds(0, R)], send_sems.at[1])
            wait_total(sendb.at[pl.ds(0, ZL)], send_sems.at[0])
            z_tail().wait_send()

            @pl.when(is01)
            def _():
                z_head_f32().wait_send()

            @pl.when(jnp.logical_not(is01))
            def _():
                z_head_bf16().wait_send()

            @pl.when(is00)
            def _():
                z_head_f32().wait_recv()
                out_ref[global_rows(ZL, B), zhead] = xv[zrows, zhead] + z32[...]

        consume_x(l // B)
        y_direct(k).wait_recv()
        finish(l, n)
        consume_x((l + n) // B)
    consume_x(2 * NB + LAG)
    z_tail().wait_recv()
    finish(ZL, B, ztail)

    @pl.when(jnp.logical_not(is00))
    def _():
        z_head_bf16().wait_recv()
        finish(ZL, B, zhead)


def pallas_dist_ar_xy_y_m1024_n512_kernel(x: jax.Array):
    return pl.pallas_call(
        _body,
        out_shape=jax.ShapeDtypeStruct((M, N), jnp.float32),
        in_specs=[pl.BlockSpec(memory_space=pl.ANY)],
        out_specs=pl.BlockSpec(memory_space=pltpu.VMEM),
        scratch_shapes=[
            pltpu.VMEM((M, N), jnp.float32),
            pltpu.VMEM((T0, N), jnp.bfloat16),
            pltpu.VMEM((M, N), jnp.bfloat16),
            pltpu.VMEM((B, CW), jnp.float32),
            pltpu.VMEM((B, ZC), jnp.float32),
            pltpu.SemaphoreType.DMA((len(LOADS) + 1,)),
            pltpu.SemaphoreType.DMA((4,)),
            pltpu.SemaphoreType.DMA((NB * NCW + len(DIRECT) + 2,)),
            pltpu.SemaphoreType.DMA((len(XGROUPS),)),
            pltpu.SemaphoreType.REGULAR,
        ],
        compiler_params=pltpu.CompilerParams(
            collective_id=0,
            disable_semaphore_checks=True,
        ),
    )(x)
```
